```python
import numpy as np

kernel_name = "dist_sort_i_m128_n64"

def setup_inputs():
    return {"x": np.random.randn(512, 64).astype(np.float32)}

def reference(x: np.ndarray) -> np.ndarray:
    return np.sort(x, axis=0)
```

```python
import jax
import jax.numpy as jnp
from jax import lax
from jax.experimental import pallas as pl
from jax.experimental.pallas import tpu as pltpu

N_DEV = 4


def _bitonic_sort_rows(x):
    n = x.shape[0]
    row = lax.broadcasted_iota(jnp.int32, x.shape, 0)
    k = 2
    while k <= n:
        j = k // 2
        while j >= 1:
            low = (row & j) == 0
            partner = jnp.where(low, pltpu.roll(x, n - j, 0), pltpu.roll(x, j, 0))
            asc = (row & k) == 0
            x = jnp.where(low == asc, jnp.minimum(x, partner), jnp.maximum(x, partner))
            j //= 2
        k *= 2
    return x


def pallas_dist_sort_i_m128_n64_kernel(x: jax.Array):
    m, n = x.shape

    def kernel_body(x_ref, o_ref, gathered, result, send_sems, recv_sems):
        me = lax.axis_index("i")
        barrier = pltpu.get_barrier_semaphore()
        for d in range(1, N_DEV):
            pl.semaphore_signal(barrier, inc=1, device_id=((me + d) % N_DEV,),
                                device_id_type=pl.DeviceIdType.MESH)
        gathered[0] = x_ref[...]
        pl.semaphore_wait(barrier, N_DEV - 1)
        copies = []
        for d in range(1, N_DEV):
            c = pltpu.make_async_remote_copy(
                src_ref=gathered.at[0], dst_ref=gathered.at[d],
                send_sem=send_sems.at[d - 1], recv_sem=recv_sems.at[d - 1],
                device_id=((me + d) % N_DEV,), device_id_type=pl.DeviceIdType.MESH)
            c.start()
            copies.append(c)
        for c in copies:
            c.wait()
        allx = jnp.concatenate([gathered[d].T for d in range(N_DEV)], axis=0)
        result[...] = _bitonic_sort_rows(allx)
        o_ref[...] = result[pl.ds(pl.multiple_of(me * m, m), m), :].T

    out_t = pl.pallas_call(
        kernel_body,
        out_shape=jax.ShapeDtypeStruct((n, m), x.dtype),
        scratch_shapes=[
            pltpu.VMEM((N_DEV, n, m), x.dtype),
            pltpu.VMEM((N_DEV * m, n), x.dtype),
            pltpu.SemaphoreType.DMA((N_DEV - 1,)),
            pltpu.SemaphoreType.DMA((N_DEV - 1,)),
        ],
        compiler_params=pltpu.CompilerParams(collective_id=0),
    )(x.T)
    return out_t.T
```

```python
import jax
import jax.numpy as jnp
from jax import lax
from jax.experimental import pallas as pl
from jax.experimental.pallas import tpu as pltpu

F32 = jnp.float32
VREG = (8, 128)

_TAKE_ROWS = lax.GatherDimensionNumbers(
    offset_dims=(), collapsed_slice_dims=(0,), start_index_map=(0,),
    operand_batching_dims=(1,), start_indices_batching_dims=(1,))


def take_rows(x, idx):
    return lax.gather(x, idx.reshape(*VREG, 1), _TAKE_ROWS, (1, 1),
                      mode=lax.GatherScatterMode.PROMISE_IN_BOUNDS)


class Consts:
    def __init__(self):
        self.sub = lax.broadcasted_iota(jnp.int32, VREG, 0)
        self.lane = lax.broadcasted_iota(jnp.int32, VREG, 1)
        self.sub_low = [(self.sub & (1 << j)) == 0 for j in range(3)]
        self.lane_bit = {j: (self.lane & (1 << j)) != 0 for j in (0, 1, 2, 6)}
        self.xor = {d: self.sub ^ d for d in range(1, 8)}

    def flip(self, x, d):
        if d == 4:
            return pltpu.roll(x, 4, 0)
        return take_rows(x, self.xor[d])


def to_key(x):
    top = 2.0 ** 127
    return jnp.where(x != x, jnp.inf, lax.clamp(-top, x * 0.5, top))


def from_key(k):
    return jnp.where(k == jnp.inf, jnp.nan, k * 2.0)


def pack(a, b):
    return pltpu.bitcast(jnp.concatenate([a, b], axis=0).astype(jnp.bfloat16), jnp.uint32)


def unpack(w):
    v = pltpu.bitcast(w, jnp.bfloat16).astype(F32)
    return v[:8], v[8:]


def group_of_tile(t):
    return 2 * (t % 4) + t // 4


def skew_half(c, tiles, parity):
    p = []
    for i, x in enumerate(tiles):
        b = 2 * i + parity
        p.append(take_rows(x, (c.sub + ((c.lane + 7 - b) >> 3)) & 7))
    p = [jnp.where(c.lane_bit[2], p[(i + 2) % 4], p[i]) for i in range(4)]
    return [jnp.where(c.lane_bit[1], p[(i + 1) % 4], p[i]) for i in range(4)]


def to_lanes(c, u, rows):
    out = []
    for a in rows:
        y = jnp.where(c.lane_bit[0], u[(a + 1) % 8], u[a])
        out += [pltpu.roll(y, a + half, 1, stride=8, stride_axis=0) for half in (0, 64)]
    return out


def cx(a, b, descending=False):
    lo, hi = jnp.minimum(a, b), jnp.maximum(a, b)
    return (hi, lo) if descending else (lo, hi)


def oe_merge(a, b):
    if not a or not b:
        return a + b
    if len(a) == 1 and len(b) == 1:
        return list(cx(a[0], b[0]))
    e, o = oe_merge(a[0::2], b[0::2]), oe_merge(a[1::2], b[1::2])
    out = [e[0]]
    n = min(len(o), len(e) - 1)
    for i in range(n):
        out += cx(o[i], e[i + 1])
    return out + o[n:] + e[n + 1:]


def oe_sort(v):
    if len(v) == 1:
        return v
    h = len(v) // 2
    return oe_merge(oe_sort(v[:h]), oe_sort(v[h:]))


def vreg_stage(v, dist, descending=False):
    v = list(v)
    for i in range(len(v)):
        if not i & dist:
            v[i], v[i + dist] = cx(v[i], v[i + dist], descending)
    return v


def split_stage(c, v, j, dist=1, descending=False):
    v = list(v)
    for i in range(len(v)):
        if not i & dist:
            a, b = v[i], v[i + dist]
            t = jnp.where(c.sub_low[j], a, b)
            u = c.flip(jnp.where(c.sub_low[j], b, a), 1 << j)
            v[i], v[i + dist] = cx(t, u, descending)
    return v


def sublane_stage(c, v, j, descending=False):
    return [jnp.where(c.sub_low[j], *cx(x, c.flip(x, 1 << j), descending)) for x in v]


def sort_lanes(c, v, order=(0, 1, 2)):
    v = oe_sort(v)
    for k in range(3):
        d = sum(1 << j for j in order[:k + 1])
        v = oe_merge(v[0::2], [c.flip(x, d) for x in v[1::2]])
        for j in order[:k + 1]:
            v = split_stage(c, v, j)
    return v


def reverse(c, v):
    return [c.flip(x, 7) for x in v[::-1]]


def bitonic_merge(c, v, descending=False):
    for d in (8, 4, 2):
        v = vreg_stage(v, d, descending)
    for j in range(3):
        v = sublane_stage(c, v, j, descending)
    return vreg_stage(v, 1, descending)


def swap_bit0_sub0(c, v):
    out = []
    for a, b in zip(v[0::2], v[1::2]):
        out += [jnp.where(c.sub_low[0], a, c.flip(b, 1)), jnp.where(c.sub_low[0], c.flip(a, 1), b)]
    return out


def absorb(c, s_desc, run):
    run = swap_bit0_sub0(c, run)
    v = [jnp.minimum(a, b) for a, b in zip(s_desc, run)] + s_desc[len(run):]
    for d in (8, 4, 2, 1):
        v = vreg_stage(v, d, True)
    for j in (1, 2, 0):
        v = split_stage(c, v, j, descending=True)
    return v


class OutConsts:
    def __init__(self, c, order):
        r5, r4, r3 = order
        sigma = (((c.sub >> r5) & 1) << 2) | (((c.sub >> r4) & 1) << 1) | ((c.sub >> r3) & 1)
        def where_is(g):
            return (((g >> 2) & 1) << r5) | (((g >> 1) & 1) << r4) | ((g & 1) << r3)
        self.upper = [(c.lane + ((8 * sigma + b - c.lane) & 63)) & 64 for b in range(8)]
        self.before = [where_is(c.sub + ((c.lane + a) >> 3)) for a in range(8)]
        self.after = [(((c.lane + 128 - a) >> 3) - c.sub) & 7 for a in range(8)]


def shift8(c, v):
    for j in (2, 1, 0):
        v = [jnp.where(c.lane_bit[j], v[(i + (1 << j)) % 8], v[i]) for i in range(8)]
    return v


def finish(c, oc, v, order=(0, 1, 2)):
    for d in (8, 4, 2):
        v = vreg_stage(v, d)
    for j, d in zip(order, (4, 2, 4)):
        v = split_stage(c, v, j, d)
    v = vreg_stage(v, 1)
    slot = lambda b: (b & 1) | ((b & 2) << 1) | ((b & 4) >> 1)
    r = [jnp.where(oc.upper[b] != 0, v[8 + slot(b)], v[slot(b)]) for b in range(8)]
    g = shift8(c, r)
    f = [pltpu.roll(take_rows(g[a], oc.before[a]), a, 1, stride=8, stride_axis=0) for a in range(8)]
    q = shift8(c, [take_rows(from_key(f[a]), oc.after[a]) for a in range(8)])
    return [q[-group_of_tile(t) % 8] for t in range(8)]


def pack_run(c, v):
    d = [jnp.where(c.lane_bit[6], v[i + 8], v[i]) for i in range(8)]
    return [pack(d[2 * i], d[2 * i + 1]) for i in range(4)]


def unpack_run(c, words):
    lo, hi = [], []
    for w in words:
        r = pltpu.roll(w, 64, 1)
        lo += unpack(jnp.where(c.lane_bit[6], r, w))
        hi += unpack(jnp.where(c.lane_bit[6], w, r))
    return lo + hi


def interleave(even, odd):
    return [x for pair in zip(even, odd) for x in pair]


MESH = pl.DeviceIdType.MESH
ROOT, FAR = 0, 2

import contextlib
def make(mode="g", idtype=MESH, prof=False, **cp):
    sc = (lambda n: jax.named_scope(n)) if prof else (lambda n: contextlib.nullcontext())
    def kernel(x):
        m, n = x.shape
        def dev(d):
            return dict(device_id=(d,), device_id_type=MESH) if idtype is MESH else dict(device_id=d, device_id_type=idtype)

        def body(x_hbm, o_ref, x_vmem, own, mine, runs, raw, half_src, half_dst, tables,
                 load_sem, send_sems, recv_sems, far_send, far_recv, near_in, far_in):
            me = lax.axis_index("i")
            barrier = pltpu.get_barrier_semaphore()

            def run_copy(slot, dst):
                return pltpu.make_async_remote_copy(mine, runs.at[slot], send_sems.at[slot], recv_sems.at[slot], **dev(dst))
            raw_copy = pltpu.make_async_remote_copy(x_hbm.at[pl.ds(0, 32)], raw, far_send.at[0], far_recv.at[0], **dev(ROOT))
            if mode == "g":
                half_copies = [pltpu.make_async_remote_copy(half_src.at[i], half_dst.at[i], far_send.at[1 + i], far_recv.at[1 + i], **dev(ROOT)) for i in range(2)]
            else:
                half_copies = [pltpu.make_async_remote_copy(half_src, half_dst, far_send.at[1], far_recv.at[1], **dev(ROOT))]
            loads = [pltpu.make_async_copy(x_hbm.at[pl.ds(32 * i, 32)], x_vmem.at[pl.ds(32 * i, 32)], load_sem.at[i]) for i in range(2)]

            @pl.when(me == ROOT)
            def _():
                for d in (FAR, 1, 3):
                    pl.semaphore_signal(barrier, inc=1, **dev(d))

            @pl.when(me != ROOT)
            def _():
                pl.semaphore_wait(barrier, 1)

            @pl.when(me == FAR)
            def _():
                raw_copy.start()

            loads[1].start()
            loads[0].start()

            @pl.when(me == FAR)
            def _():
                pl.semaphore_signal(far_in, inc=1, **dev(ROOT))

            @pl.when(me & 1 == 1)
            def _():
                pl.semaphore_signal(near_in, inc=1, **dev(ROOT))

            c = Consts()
            with sc("w_ld1"): loads[1].wait()
            odd = skew_half(c, [to_key(x_vmem[8 * t:8 * t + 8]) for t in range(4, 8)], 1)
            half_src[0] = pack(odd[0], odd[1])
            half_src[1] = pack(odd[2], odd[3])

            @pl.when(me == FAR)
            def _():
                for h in half_copies:
                    h.start()

            with sc("w_ld0"): loads[0].wait()
            even = skew_half(c, [to_key(x_vmem[8 * t:8 * t + 8]) for t in range(4)], 0)
            run = sort_lanes(c, to_lanes(c, interleave(even, odd), range(8)))
            for i, w in enumerate(pack_run(c, run)):
                mine[i] = w
            for i, v in enumerate(run):
                own[i] = v

            def received(slot):
                run_copy(slot, ROOT).wait_recv()
                return unpack_run(c, [runs[slot, i] for i in range(4)])

            @pl.when(me != ROOT)
            def _():
                @pl.when(me == FAR)
                def _():
                    pl.semaphore_wait(barrier, 1)
                    run_copy(0, 3).start()
                    run_copy(2, 1).start()
                    raw_copy.wait_send()
                    for h in half_copies:
                        h.wait_send()

                for pos in (1, 3):
                    @pl.when(me == pos)
                    def _():
                        run_copy((ROOT - pos) % 4 - 1, ROOT).start()
                        pl.semaphore_wait(near_in, 1)
                        run_copy(1, 4 - pos).start()
                        with sc("w_far"): pl.semaphore_wait(far_in, 1)
                        run_copy((FAR - pos) % 4 - 1, FAR).start()
                        run_copy(1, ROOT).wait_send()

                def merge2(a, b, desc):
                    lo, hi = zip(*[cx(p, q) for p, q in zip(a, reverse(c, b))])
                    lo, hi = bitonic_merge(c, lo, desc), bitonic_merge(c, hi, desc)
                    return hi + lo if desc else lo + hi
                first = me - 1
                p = merge2([own[i] for i in range(16)], received(first), False)
                a, b = (first + 1) % 3, (first + 2) % 3
                run_copy(a, ROOT).wait_recv()
                run_copy(b, ROOT).wait_recv()
                q = merge2(*[unpack_run(c, [runs[slot, i] for i in range(4)]) for slot in (a, b)], True)
                v = [jnp.where(me < 2, *cx(s, t)) for s, t in zip(p, q)]
                w = [jnp.where(me == 2, *cx(v[i], v[i + 16])) for i in range(16)]
                for t, tile in enumerate(finish(c, OutConsts(c, (0, 1, 2)), w)):
                    o_ref[8 * t:8 * t + 8] = tile
                run_copy(0, ROOT).wait_send()
                run_copy(2, ROOT).wait_send()

            @pl.when(me == ROOT)
            def _():
                order = (1, 2, 0) if mode == "g" else (0, 1, 2)
                oc = OutConsts(c, order)
                for i, t in enumerate(oc.upper + oc.before + oc.after):
                    tables[i] = t
                with sc("w_near"): pl.semaphore_wait(near_in, 2)
                pl.semaphore_signal(barrier, inc=1, **dev(FAR))
                for d in (1, 3):
                    pl.semaphore_signal(near_in, inc=1, **dev(d))
                run_copy(0, 1).start()
                run_copy(2, 3).start()
                with sc("w_far"): pl.semaphore_wait(far_in, 1)
                run_copy(1, FAR).start()
                for d in (1, 3):
                    pl.semaphore_signal(far_in, inc=1, **dev(d))
                s = reverse(c, [own[i] for i in range(16)])
                with sc("w_r0"): run_copy(0, ROOT).wait_recv()
                with sc("w_r2"): run_copy(2, ROOT).wait_recv()
                b, d = [unpack_run(c, [runs[slot, i] for i in range(4)]) for slot in (0, 2)]
                s = bitonic_merge(c, [jnp.minimum(p, q) for p, q in zip(s, b)], True)
                s = bitonic_merge(c, [jnp.minimum(p, q) for p, q in zip(s, d)], True)
                if mode == "g":
                    s = swap_bit0_sub0(c, s)
                for i, v in enumerate(s):
                    own[i] = v
                for slot in range(3):
                    with sc("w_snd"): run_copy(slot, ROOT).wait_send()
                with sc("w_raw"): raw_copy.wait_recv()
                ev = skew_half(c, [to_key(raw[8 * t:8 * t + 8]) for t in range(4)], 0)
                if mode == "g":
                    u = interleave(ev, [None] * 4)
                    with sc("w_h0"): half_copies[0].wait_recv()
                    u[1], u[3] = unpack(half_dst[0])
                    z1 = to_lanes(c, u, range(4))
                    with sc("w_h1"): half_copies[1].wait_recv()
                    u[5], u[7] = unpack(half_dst[1])
                    z2 = to_lanes(c, u, range(4, 8))
                    s = absorb(c, [own[i] for i in range(16)], sort_lanes(c, z1))
                    e2 = sort_lanes(c, z2, order)
                    v = [jnp.minimum(p, q) for p, q in zip(s, e2)] + s[8:]
                else:
                    with sc("w_h0"): half_copies[0].wait_recv()
                    od = [*unpack(half_dst[0]), *unpack(half_dst[1])]
                    e = sort_lanes(c, to_lanes(c, interleave(ev, od), (0, 2, 4, 6, 1, 3, 5, 7)))
                    v = [jnp.minimum(own[i], e[i]) for i in range(16)]
                oc.upper = [tables[i] for i in range(8)]
                oc.before = [tables[8 + i] for i in range(8)]
                oc.after = [tables[16 + i] for i in range(8)]
                for t, tile in enumerate(finish(c, oc, v, order)):
                    o_ref[8 * t:8 * t + 8] = tile

        u32 = jnp.uint32
        return pl.pallas_call(
            body, name="dsort",
            out_shape=jax.ShapeDtypeStruct((n, m), x.dtype),
            in_specs=[pl.BlockSpec(memory_space=pltpu.HBM)],
            out_specs=pl.BlockSpec(memory_space=pltpu.VMEM),
            scratch_shapes=[
                pltpu.VMEM((n, m), F32), pltpu.VMEM((16, *VREG), F32), pltpu.VMEM((4, *VREG), u32),
                pltpu.VMEM((3, 4, *VREG), u32), pltpu.VMEM((n // 2, m), F32),
                pltpu.VMEM((2, *VREG), u32), pltpu.VMEM((2, *VREG), u32), pltpu.VMEM((24, *VREG), jnp.int32),
                pltpu.SemaphoreType.DMA((2,)), pltpu.SemaphoreType.DMA((3,)), pltpu.SemaphoreType.DMA((3,)),
                pltpu.SemaphoreType.DMA((3,)), pltpu.SemaphoreType.DMA((3,)),
                pltpu.SemaphoreType.REGULAR, pltpu.SemaphoreType.REGULAR,
            ],
            compiler_params=pltpu.CompilerParams(collective_id=0, disable_semaphore_checks=True, **cp),
        )(x.T).T
    return kernel


def pallas_dist_sort_i_m128_n64_kernel(x):
    return make('g')(x)
```

```python
import jax
import jax.numpy as jnp
from jax import lax
from jax.experimental import pallas as pl
from jax.experimental.pallas import tpu as pltpu

ROOT, FAR, NEAR = 0, 2, (1, 3)
VREG = (8, 128)
GROUP = (0, 1, 4, 5, 2, 3, 6, 7)
RAW_ROWS = 24
PLAIN, ROTATED = (0, 1, 2), (1, 2, 0)

_KEY_INF = 2.0 ** 127
_KEY_MAX = _KEY_INF * (1.0 - 2.0 ** -8)

_TAKE_ROWS = lax.GatherDimensionNumbers(
    offset_dims=(), collapsed_slice_dims=(0,), start_index_map=(0,),
    operand_batching_dims=(1,), start_indices_batching_dims=(1,))


def _to_key(x):
    special = jnp.where(x != x, jnp.inf, lax.clamp(-_KEY_INF, x, _KEY_INF))
    return jnp.where(jnp.abs(x) < jnp.inf, lax.clamp(-_KEY_MAX, x * 0.5, _KEY_MAX), special)


def _from_key(k):
    return jnp.where(k == jnp.inf, jnp.nan, k * 2.0)


def _store_packed(ref, regs):
    for i, x in enumerate(regs):
        ref[pl.ds(4 * i, 4)] = pltpu.bitcast(x.astype(jnp.bfloat16), jnp.uint32)


def _unpack(words):
    x = pltpu.bitcast(words, jnp.bfloat16).astype(jnp.float32)
    return [x[i:i + 8] for i in range(0, x.shape[0], 8)]


def _take_rows(x, rows):
    return lax.gather(x, rows.reshape(*VREG, 1), _TAKE_ROWS, (1, 1),
                      mode=lax.GatherScatterMode.PROMISE_IN_BOUNDS)


def _rotate(x, shift):
    return pltpu.roll(x, shift, 1, stride=8, stride_axis=0)


def _to_lanes(rows, shifts):
    return [_rotate(y, a + half) for y, a in zip(rows, shifts) for half in (0, 64)]


def _order(a, b, descending=False):
    lo, hi = jnp.minimum(a, b), jnp.maximum(a, b)
    return (hi, lo) if descending else (lo, hi)


def _merge_regs(a, b):
    if not a or not b:
        return a + b
    if len(a) == 1 and len(b) == 1:
        return list(_order(a[0], b[0]))
    even, odd = _merge_regs(a[0::2], b[0::2]), _merge_regs(a[1::2], b[1::2])
    n = min(len(odd), len(even) - 1)
    out = [even[0]]
    for i in range(n):
        out += _order(odd[i], even[i + 1])
    return out + odd[n:] + even[n + 1:]


def _sort_regs(v):
    if len(v) == 1:
        return v
    return _merge_regs(_sort_regs(v[:len(v) // 2]), _sort_regs(v[len(v) // 2:]))


def _reg_stage(v, dist, descending=False):
    v = list(v)
    for i in range(len(v)):
        if not i & dist:
            v[i], v[i + dist] = _order(v[i], v[i + dist], descending)
    return v


def _lowest(descending_run, ascending_run):
    low = [jnp.minimum(a, b) for a, b in zip(descending_run, ascending_run)]
    return low + descending_run[len(low):]


class _Lanes:
    def __init__(self):
        self.sub = lax.broadcasted_iota(jnp.int32, VREG, 0)
        self.lane = lax.broadcasted_iota(jnp.int32, VREG, 1)
        self.sub_clear = [(self.sub & (1 << j)) == 0 for j in range(3)]
        self.lane_set = {j: (self.lane & (1 << j)) != 0 for j in (0, 1, 2, 6)}
        self.sub_xor = {d: self.sub ^ d for d in (1, 2, 3, 6, 7)}

    def flip(self, x, d):
        return pltpu.roll(x, 4, 0) if d == 4 else _take_rows(x, self.sub_xor[d])

    def pick(self, j, clear, set_):
        return jnp.where(self.lane_set[j], set_, clear)

    def shift_regs(self, v):
        for j in (2, 1, 0):
            v = [self.pick(j, v[a], v[(a + (1 << j)) % 8]) for a in range(8)]
        return v

    def skew_rows(self, tile):
        return (self.sub + ((self.lane + (7 - GROUP[tile])) >> 3)) & 7

    def split_in_halves(self, tiles):
        v = [self.pick(2, tiles[i], tiles[i ^ 2]) for i in range(4)]
        v = [self.pick(0, v[i], v[i ^ 1]) for i in range(4)]
        return v[0::2], v[1::2]

    def odd_rotation_inputs(self, pair):
        late, early = (self.lane & 3) >= 3, (self.lane & 3) >= 1
        return [jnp.where(m, q, p) for p, q in (pair, pair[::-1]) for m in (late, early)]

    def trade_stage(self, v, j, dist=1, descending=False):
        v = list(v)
        for i in range(len(v)):
            if not i & dist:
                a, b = v[i], v[i + dist]
                other = self.flip(jnp.where(self.sub_clear[j], b, a), 1 << j)
                v[i], v[i + dist] = _order(jnp.where(self.sub_clear[j], a, b), other, descending)
        return v

    def merge_sublanes(self, v, order, keep=lambda v: v):
        for k in range(3):
            mirror = sum(1 << j for j in order[:k + 1])
            v = _merge_regs(v[0::2], [self.flip(x, mirror) for x in v[1::2]])
            if k == 2:
                v = keep(v)
            for j in order[:k + 1]:
                v = self.trade_stage(v, j)
        return v

    def reverse(self, v):
        return [self.flip(x, 7) for x in v[::-1]]

    def merge_bitonic(self, v, descending):
        for dist in (8, 4, 2):
            v = _reg_stage(v, dist, descending)
        for j in PLAIN:
            v = [jnp.where(self.sub_clear[j], *_order(x, self.flip(x, 1 << j), descending))
                 for x in v]
        return _reg_stage(v, 1, descending)

    def merge_runs(self, a, b, descending):
        lo, hi = zip(*map(_order, a, self.reverse(b)))
        lo, hi = self.merge_bitonic(lo, descending), self.merge_bitonic(hi, descending)
        return hi + lo if descending else lo + hi

    def top_bits_to_regs(self, v):
        out = []
        for a, b in zip(v[0::2], v[1::2]):
            out += [jnp.where(self.sub_clear[0], a, self.flip(b, 1)),
                    jnp.where(self.sub_clear[0], self.flip(a, 1), b)]
        return out

    def share_out(self, j, v):
        return [self.pick(j, a, b) for a, b in zip(v, v[len(v) // 2:])]

    def unpack_run(self, words):
        lo, hi = [], []
        for w in words:
            other = pltpu.roll(w, 64, 1)
            lo += _unpack(self.pick(6, w, other))
            hi += _unpack(self.pick(6, other, w))
        return lo + hi

    def output_tables(self, order):
        p, q, r = order
        mid = (((self.sub >> p) & 1) << 2) | (((self.sub >> q) & 1) << 1) | ((self.sub >> r) & 1)
        upper = [(self.lane + ((8 * mid + b - self.lane) & 63)) & 64 for b in range(8)]
        wanted = [self.sub + ((self.lane + a) >> 3) for a in range(8)]
        before = [(((g >> 2) & 1) << p) | (((g >> 1) & 1) << q) | ((g & 1) << r) for g in wanted]
        after = [(((self.lane + 128 - a) >> 3) - self.sub) & 7 for a in range(8)]
        return upper + before + after

    def to_tiles(self, v, order, tables):
        for dist in (8, 4, 2):
            v = _reg_stage(v, dist)
        for j, dist in zip(order, (4, 2, 4)):
            v = self.trade_stage(v, j, dist)
        v = _reg_stage(v, 1)
        low = [(b & 1) | ((b & 2) << 1) | ((b & 4) >> 1) for b in range(8)]
        v = [jnp.where(tables[b] != 0, v[8 + low[b]], v[low[b]]) for b in range(8)]
        v = [_rotate(_take_rows(x, tables[8 + a]), a) for a, x in enumerate(self.shift_regs(v))]
        v = self.shift_regs([_take_rows(_from_key(x), tables[16 + a]) for a, x in enumerate(v)])
        return [v[-g % 8] for g in GROUP]


def _slot(src, dst):
    return [d for d in (ROOT, *NEAR, FAR) if d != dst].index(src)


def _kernel_body(x_hbm, out_ref, x_vmem, own, run_out, runs_in, raw_in,
                 tile_out, tile_in, unsorted_out, unsorted_in, sorted_out, sorted_in,
                 load_sems, run_send, run_recv, piece_send, piece_recv, near_ready, far_ready):
    def chip(d):
        return dict(device_id=(d,), device_id_type=pl.DeviceIdType.MESH)

    def run_copy(src, dst):
        return pltpu.make_async_remote_copy(
            run_out, runs_in.at[_slot(src, dst)],
            run_send.at[_slot(dst, src)], run_recv.at[_slot(src, dst)], **chip(dst))

    def rows(t):
        return pl.ds(8 * t, 8)

    raw_rows, other_rows = pl.ds(0, RAW_ROWS), pl.ds(RAW_ROWS, 64 - RAW_ROWS)
    load_raw, load_other = [
        pltpu.make_async_copy(x_hbm.at[r], x_vmem.at[r], load_sems.at[i])
        for i, r in enumerate((raw_rows, other_rows))]
    pieces = [
        pltpu.make_async_remote_copy(src, dst, piece_send.at[i], piece_recv.at[i], **chip(ROOT))
        for i, (src, dst) in enumerate((
            (x_hbm.at[raw_rows], raw_in), (tile_out, tile_in),
            (unsorted_out, unsorted_in), (sorted_out, sorted_in)))]
    raw_copy, tile_copy, unsorted_copy, sorted_copy = pieces

    load_other.start()
    me = lax.axis_index("i")
    barrier = pltpu.get_barrier_semaphore()

    @pl.when(me == FAR)
    def _stream_to_root():
        pl.semaphore_wait(barrier, 1)
        raw_copy.start()
        pl.semaphore_signal(far_ready, inc=1, **chip(ROOT))
        lanes = _Lanes()
        skew = {t: lanes.skew_rows(t) for t in range(4, 8)}
        sorted_out[...] = pltpu.bitcast((lanes.sub + ((lanes.lane >> 1) & 1)) & 7, jnp.uint32)

        load_other.wait()
        even, odd = lanes.split_in_halves(
            [_take_rows(x_vmem[rows(t)], skew[t]) for t in range(4, 8)])
        _store_packed(tile_out, [_to_key(x_vmem[rows(3)])])
        tile_copy.start()
        _store_packed(unsorted_out, map(_to_key, odd))
        unsorted_copy.start()
        wrapped = pltpu.bitcast(sorted_out[...], jnp.int32)
        p, q = map(_to_key, even)
        half = _to_lanes(
            [p, lanes.pick(1, p, q), q, _take_rows(lanes.pick(1, q, p), wrapped)], (0, 2, 4, 6))
        half = _merge_regs(_sort_regs(half[:6]), _sort_regs(half[6:]))
        _store_packed(sorted_out, lanes.merge_sublanes(
            half, ROTATED, lambda v: lanes.share_out(1, lanes.share_out(6, v))))
        sorted_copy.start()
        load_raw.start()

    @pl.when(me != FAR)
    def _check_in():
        load_raw.start()

        @pl.when(me == ROOT)
        def _():
            for d in (FAR, *NEAR):
                pl.semaphore_signal(barrier, inc=1, **chip(d))

        @pl.when(me != ROOT)
        def _():
            pl.semaphore_wait(barrier, 1)
            pl.semaphore_signal(near_ready, inc=1, **chip(ROOT))

        load_other.wait()

    lanes = _Lanes()
    skew = [lanes.skew_rows(t) for t in range(8)]
    load_raw.wait()
    tiles = [_take_rows(_to_key(x_vmem[rows(t)]), skew[t]) for t in range(8)]
    run = _to_lanes(lanes.shift_regs([tiles[GROUP.index(g)] for g in range(8)]), range(8))
    run = lanes.merge_sublanes(_sort_regs(run), PLAIN)
    _store_packed(run_out, lanes.share_out(6, run))
    for i, v in enumerate(run):
        own[i] = v

    def own_run():
        return [own[i] for i in range(16)]

    def received_run(slot):
        return lanes.unpack_run([runs_in[slot, rows(i)] for i in range(4)])

    @pl.when(me != ROOT)
    def _others():
        @pl.when(me == FAR)
        def _():
            pl.semaphore_wait(barrier, 1)
            copies = [run_copy(FAR, d) for d in NEAR]
            for copy in copies:
                copy.start()
            for copy in pieces + copies:
                copy.wait_send()

        for near, other in (NEAR, NEAR[::-1]):
            @pl.when(me == near)
            def _():
                copies = [run_copy(near, d) for d in (ROOT, other, FAR)]
                copies[0].start()
                pl.semaphore_wait(near_ready, 1)
                copies[1].start()
                pl.semaphore_wait(far_ready, 1)
                copies[2].start()
                for copy in copies:
                    copy.wait_send()

        tables = lanes.output_tables(PLAIN)
        arrivals = [run_copy(src, FAR) for src in (ROOT, *NEAR)]
        arrivals[0].wait_recv()
        up = lanes.merge_runs(own_run(), received_run(0), False)
        arrivals[1].wait_recv()
        arrivals[2].wait_recv()
        down = lanes.merge_runs(received_run(1), received_run(2), True)
        half = [jnp.where(me < 2, *_order(a, b)) for a, b in zip(up, down)]
        quarter = [jnp.where(me == 2, *_order(half[i], half[i + 16])) for i in range(16)]
        for t, tile in enumerate(lanes.to_tiles(quarter, PLAIN, tables)):
            out_ref[rows(t)] = tile

    @pl.when(me == ROOT)
    def _root():
        tables = lanes.output_tables(ROTATED)
        copies = [run_copy(ROOT, d) for d in (*NEAR, FAR)]
        pl.semaphore_wait(near_ready, 2)
        pl.semaphore_signal(barrier, inc=1, **chip(FAR))
        for d in NEAR:
            pl.semaphore_signal(near_ready, inc=1, **chip(d))
        copies[0].start()
        copies[1].start()
        pl.semaphore_wait(far_ready, 1)
        copies[2].start()
        for d in NEAR:
            pl.semaphore_signal(far_ready, inc=1, **chip(d))

        best = lanes.reverse(own_run())
        for d in NEAR:
            run_copy(d, ROOT).wait_recv()
        for run in [received_run(_slot(d, ROOT)) for d in NEAR]:
            best = lanes.merge_bitonic(_lowest(best, run), True)
        for i, v in enumerate(lanes.top_bits_to_regs(best)):
            own[i] = v
        for copy in copies:
            copy.wait_send()

        raw_copy.wait_recv()
        tiles = [_take_rows(_to_key(raw_in[rows(t)]), skew[t]) for t in range(3)]
        tile_copy.wait_recv()
        tiles.append(_take_rows(*_unpack(tile_in[...]), skew[3]))
        even, odd = lanes.split_in_halves(tiles)
        last = _to_lanes([even[0], even[1], even[1], even[0]], (0, 2, 4, 6))
        odd = lanes.odd_rotation_inputs(odd)
        from_words = [((lanes.lane + a) & 2) != 0 for a in (1, 3, 5, 7)]

        unsorted_copy.wait_recv()
        words = lanes.odd_rotation_inputs(_unpack(unsorted_in[...]))
        first = _to_lanes(map(jnp.where, from_words, words, odd), (1, 3, 5, 7))
        last = lanes.merge_sublanes(_sort_regs(last), ROTATED)
        early = _sort_regs(first[:6])

        sorted_copy.wait_recv()
        w0 = sorted_in[...]
        w2, w64, w66 = [pltpu.roll(w0, shift, 1) for shift in (2, 64, 66)]
        first = lanes.merge_sublanes(_merge_regs(early, _sort_regs(first[6:])), PLAIN)
        best = _lowest(own_run(), lanes.top_bits_to_regs(first))
        for dist in (8, 4, 2, 1):
            best = _reg_stage(best, dist, True)
        for j in ROTATED:
            best = lanes.trade_stage(best, j, descending=True)
        sent = [v for pair in ((w2, w66), (w0, w64), (w66, w2), (w64, w0))
                for v in _unpack(lanes.pick(6, *pair))]
        last = [lanes.pick(1, a, b) for a, b in zip(last, sent)]
        for t, tile in enumerate(lanes.to_tiles(_lowest(best, last), ROTATED, tables)):
            out_ref[rows(t)] = tile


def pallas_dist_sort_i_m128_n64_kernel(x: jax.Array):
    assert x.shape == (128, 64), x.shape
    f32, u32 = jnp.float32, jnp.uint32
    dma, regular = pltpu.SemaphoreType.DMA, pltpu.SemaphoreType.REGULAR
    out_t = pl.pallas_call(
        _kernel_body,
        out_shape=jax.ShapeDtypeStruct((64, 128), f32),
        in_specs=[pl.BlockSpec(memory_space=pltpu.HBM)],
        out_specs=pl.BlockSpec(memory_space=pltpu.VMEM),
        scratch_shapes=[
            pltpu.VMEM((64, 128), f32),
            pltpu.VMEM((16, *VREG), f32),
            pltpu.VMEM((32, 128), u32),
            pltpu.VMEM((3, 32, 128), u32),
            pltpu.VMEM((RAW_ROWS, 128), f32),
            pltpu.VMEM((4, 128), u32),
            pltpu.VMEM((4, 128), u32),
            pltpu.VMEM(VREG, u32),
            pltpu.VMEM(VREG, u32),
            pltpu.VMEM(VREG, u32),
            pltpu.VMEM(VREG, u32),
            dma((2,)), dma((3,)), dma((3,)), dma((4,)), dma((4,)), regular, regular,
        ],
        compiler_params=pltpu.CompilerParams(collective_id=0, disable_semaphore_checks=True),
    )(x.astype(f32).T)
    return out_t.T
```
